```python
import numpy as np

kernel_name = "dist_rmsnorm_colshard_i_m768_n512"

def setup_inputs():
    x = np.random.randn(768, 2048).astype(np.float32)
    gamma = np.random.randn(2048).astype(np.float32)
    return {"x": x, "gamma": gamma}

def reference(x: np.ndarray, gamma: np.ndarray) -> np.ndarray:
    eps = 1e-5
    rms = np.sqrt(np.mean(x * x, axis=1, keepdims=True) + eps)
    return gamma * x / rms
```

```python
import jax
import jax.numpy as jnp
from jax import lax
from jax.experimental import pallas as pl
from jax.experimental.pallas import tpu as pltpu

_N_DEV = 4
_EPS = 1e-5
_SUBLANES = 8
_LANES = 128

_GROUP_ROWS = (384, 224, 112, 48)
_FIRST_SMEM_GROUP = 2

_NEAR = (1, 3)
_FAR = 2


def pallas_dist_rmsnorm_colshard_i_m768_n512_kernel(
    x: jax.Array,
    gamma: jax.Array,
):
    m, n = x.shape
    assert sum(_GROUP_ROWS) == m and n % _LANES == 0
    n_groups = len(_GROUP_ROWS)
    row0 = [sum(_GROUP_ROWS[:g]) for g in range(n_groups)]
    n_lines = [pl.cdiv(rows, _LANES) for rows in _GROUP_ROWS]
    line0 = [sum(n_lines[:g]) for g in range(n_groups)]
    inv_cols = 1.0 / (_N_DEV * n)

    def body(x_hbm, gamma_hbm, out_ref, x_buf, gamma_buf, mine, near,
             load_sems, send_sems, near_sems, far_sems, *far):
        loads = [
            pltpu.make_async_copy(
                x_hbm.at[pl.ds(row0[g], _GROUP_ROWS[g])],
                x_buf.at[pl.ds(row0[g], _GROUP_ROWS[g])],
                load_sems.at[g],
            )
            for g in range(n_groups)
        ]
        for load in loads:
            load.start()

        me = lax.axis_index("i")
        barrier = pltpu.get_barrier_semaphore()
        for d in (_FAR,) + _NEAR:
            pl.semaphore_signal(
                barrier, inc=1, device_id=me ^ d,
                device_id_type=pl.DeviceIdType.LOGICAL,
            )

        gamma_load = pltpu.make_async_copy(
            gamma_hbm, gamma_buf, load_sems.at[n_groups]
        )
        gamma_load.start()

        far_copies = [
            pltpu.make_async_remote_copy(
                src_ref=mine.at[pl.ds(line0[g], n_lines[g])],
                dst_ref=far[g],
                send_sem=send_sems.at[g],
                recv_sem=far_sems.at[g],
                device_id=me ^ _FAR,
                device_id_type=pl.DeviceIdType.LOGICAL,
            )
            for g in range(n_groups)
        ]
        near_copies = [
            pltpu.make_async_remote_copy(
                src_ref=mine,
                dst_ref=near.at[j],
                send_sem=send_sems.at[n_groups + j],
                recv_sem=near_sems.at[j],
                device_id=me ^ d,
                device_id_type=pl.DeviceIdType.LOGICAL,
            )
            for j, d in enumerate(_NEAR)
        ]

        tile = (_SUBLANES, _LANES)
        sublane = lax.broadcasted_iota(jnp.int32, tile, 0)
        diagonal = lax.broadcasted_iota(jnp.int32, tile, 1) - sublane

        def slots(k):
            return diagonal == k % _LANES

        def rows(g, k):
            return pl.ds(row0[g] + k, _SUBLANES)

        for g in range(n_groups):
            loads[g].wait()
            packed = jnp.zeros(tile, jnp.float32)
            for k in range(0, _GROUP_ROWS[g], _SUBLANES):
                sq = jnp.square(x_buf[rows(g, k), :])
                parts = [sq[:, c:c + _LANES] for c in range(0, n, _LANES)]
                while len(parts) > 1:
                    parts = parts[2:] + [parts[0] + parts[1]]
                row_sum = jnp.sum(parts[0], axis=1, keepdims=True)
                packed = jnp.where(slots(k), row_sum, packed)
                end = k + _SUBLANES
                if end % _LANES == 0 or end == _GROUP_ROWS[g]:
                    mine[line0[g] + k // _LANES] = (
                        jnp.sum(packed, axis=0, keepdims=True) * inv_cols
                    )
                    packed = jnp.zeros(tile, jnp.float32)
            if g == 0:
                pl.semaphore_wait(barrier, _N_DEV - 1)
            far_copies[g].start()
        for copy in near_copies:
            copy.start()

        gamma_load.wait()
        gamma_tile = jnp.broadcast_to(gamma_buf[...], (_SUBLANES, n))
        for copy in far_copies + near_copies:
            copy.wait_send()
        for copy in near_copies:
            copy.wait_recv()

        def all_but_far(g, k):
            line = line0[g] + k // _LANES
            return (mine[line] + _EPS) + (near[0, line] + near[1, line])

        def unpack(line_tile, k):
            return jnp.sum(
                jnp.where(slots(k), line_tile, 0.0), axis=1, keepdims=True
            )

        partial = {}
        for g in range(_FIRST_SMEM_GROUP, n_groups):
            for k in range(0, _GROUP_ROWS[g], _SUBLANES):
                if k % _LANES == 0:
                    line_tile = jnp.broadcast_to(all_but_far(g, k), tile)
                partial[g, k] = jnp.broadcast_to(unpack(line_tile, k), tile)

        for g in range(n_groups):
            steps = range(0, _GROUP_ROWS[g], _SUBLANES)
            if g == n_groups - 1:
                ready = {k: gamma_tile * x_buf[rows(g, k), :] for k in steps}
            far_copies[g].wait_recv()
            for k in steps:
                line, slot = divmod(k, _LANES)
                if g >= _FIRST_SMEM_GROUP:
                    far_part = jnp.full(tile, far[g][line, 0, slot], jnp.float32)
                    for s in range(1, _SUBLANES):
                        far_part = jnp.where(
                            sublane == s, far[g][line, 0, slot + s], far_part
                        )
                    inv_rms = lax.rsqrt(partial[g, k] + far_part)
                    inv_rms = jnp.concatenate([inv_rms] * (n // _LANES), axis=1)
                else:
                    if slot == 0:
                        line_tile = jnp.broadcast_to(
                            lax.rsqrt(all_but_far(g, k) + far[g][line]), tile
                        )
                    inv_rms = unpack(line_tile, k)
                if g == n_groups - 1:
                    scaled = ready[k]
                else:
                    scaled = gamma_tile * x_buf[rows(g, k), :]
                out_ref[rows(g, k), :] = scaled * inv_rms

    total_lines = sum(n_lines)
    far_shapes = [
        (pltpu.SMEM if g >= _FIRST_SMEM_GROUP else pltpu.VMEM)(
            (n_lines[g], 1, _LANES), jnp.float32
        )
        for g in range(n_groups)
    ]
    return pl.pallas_call(
        body,
        out_shape=jax.ShapeDtypeStruct((m, n), x.dtype),
        in_specs=[
            pl.BlockSpec(memory_space=pltpu.HBM),
            pl.BlockSpec(memory_space=pltpu.HBM),
        ],
        out_specs=pl.BlockSpec(memory_space=pltpu.VMEM),
        scratch_shapes=[
            pltpu.VMEM((m, n), x.dtype),
            pltpu.VMEM((1, n), gamma.dtype),
            pltpu.VMEM((total_lines, 1, _LANES), jnp.float32),
            pltpu.VMEM((len(_NEAR), total_lines, 1, _LANES), jnp.float32),
            pltpu.SemaphoreType.DMA((n_groups + 1,)),
            pltpu.SemaphoreType.DMA((n_groups + len(_NEAR),)),
            pltpu.SemaphoreType.DMA((len(_NEAR),)),
            pltpu.SemaphoreType.DMA((n_groups,)),
            *far_shapes,
        ],
        compiler_params=pltpu.CompilerParams(
            collective_id=0,
            disable_semaphore_checks=True,
        ),
    )(x, gamma.reshape(1, n))
```
